```python
import numpy as np

kernel_name = "dist_mlpseq_tp2d_cs_cs_b64_d2048_h4096"

def setup_inputs():
    x = np.random.randn(64, 4096).astype(np.float32)
    Win0 = np.random.randn(4096, 8192).astype(np.float32)
    Wout0 = np.random.randn(8192, 4096).astype(np.float32)
    Win1 = np.random.randn(4096, 8192).astype(np.float32)
    Wout1 = np.random.randn(8192, 4096).astype(np.float32)
    Win2 = np.random.randn(4096, 8192).astype(np.float32)
    Wout2 = np.random.randn(8192, 4096).astype(np.float32)
    return {"x": x, "Win0": Win0, "Wout0": Wout0, "Win1": Win1, "Wout1": Wout1, "Win2": Win2, "Wout2": Wout2}

def reference(x, Win0, Win1, Win2, Wout0, Wout1, Wout2):
    h = x @ Win0
    h = np.maximum(h, 0.0)
    x = h @ Wout0
    h = x @ Win1
    h = np.maximum(h, 0.0)
    x = h @ Wout1
    h = x @ Win2
    h = np.maximum(h, 0.0)
    x = h @ Wout2
    return x
```

```python
import jax
import jax.numpy as jnp
from jax import lax
from jax.experimental import pallas as pl
from jax.experimental.pallas import tpu as pltpu

MESH = pl.DeviceIdType.MESH
B = 64
U = 1024
LANES = 128
NT = U // LANES
NSLOT = 3
NUNIT = 48


def make(LAG=14, TLAG=7, xmode="local", compute=True, f32mm=False, checks=False):
    NREG = (NUNIT - 2) * NT

    def body(x_hbm, w0, w1, w2, w3, w4, w5, obuf,
             wbuf, act, acc, sbuf, rbuf, xf,
             wsem, tsem, xsem, ssem, rsem):
        ws = (w0, w1, w2, w3, w4, w5)
        mx = lax.axis_index("x")
        my = lax.axis_index("y")

        def coords(u):
            m, v = u // 8, u % 8
            hi, lo = v // 4, v % 4
            odd = m % 2
            kb = jnp.where(odd == 1, lo, hi)
            jb = jnp.where(odd == 1, hi, lo)
            return m, odd, kb, jb

        def issue_from(w, kb, jb, slot, i):
            for t in range(2):
                for s in range(8):
                    row = s * 128 + t * 8 + i * 16
                    pltpu.make_async_copy(
                        w.at[pl.ds(pl.multiple_of(kb * U + row, 8), 8), pl.ds(pl.multiple_of(jb * U, U), U)],
                        wbuf.at[slot, pl.ds(pl.multiple_of(row, 8), 8)],
                        wsem.at[slot]).start(priority=s % 2)

        def issue(r):
            u, i = r // NT, r % NT
            m, _, kb, jb = coords(u)
            slot = u % NSLOT
            for k, w in enumerate(ws):
                pl.when(m == k)(lambda w=w: issue_from(w, kb, jb, slot, i))

        def issue_tail(q):
            n, hh = q // 2, q % 2
            slot = (NUNIT - 2 + hh) % NSLOT
            col = pl.multiple_of(n * LANES, LANES)
            for t in range(2):
                for s in range(8):
                    row = s * 128 + t * 64
                    pltpu.make_async_copy(
                        w5.at[pl.ds(pl.multiple_of((2 + hh) * U + row, 64), 64), pl.ds(pl.multiple_of(U + col, LANES), LANES)],
                        wbuf.at[slot, pl.ds(row, 64), pl.ds(col, LANES)],
                        tsem.at[q]).start(priority=s % 2)

        def first(r, _):
            issue_from(w0, 0, r // NT, r // NT, r % NT)
        lax.fori_loop(0, 2, first, None)

        bsem = pltpu.get_barrier_semaphore()
        pl.semaphore_signal(bsem, 1, device_id=(1 - mx, my), device_id_type=MESH)
        pl.semaphore_signal(bsem, 1, device_id=(mx, 1 - my), device_id_type=MESH)
        xcp = pltpu.make_async_copy(x_hbm, xf, xsem)
        xcp.start()
        lax.fori_loop(2, LAG, first, None)
        xcp.wait()
        for b in range(2):
            act[b] = xf[:, b * U:(b + 1) * U].astype(act.dtype)
        pl.semaphore_wait(bsem, 2)

        def mm(lhs, slot, n):
            w = wbuf[slot, :, pl.ds(pl.multiple_of(n * LANES, LANES), LANES)]
            if not f32mm:
                w = w.astype(jnp.bfloat16)
            return jnp.dot(act[lhs], w, preferred_element_type=jnp.float32)

        def send(e, n, sem, odd):
            tx = jnp.where(odd == 1, 1 - mx, mx)
            ty = jnp.where(odd == 1, my, 1 - my)
            pltpu.make_async_remote_copy(sbuf.at[e, n], rbuf.at[e, n], ssem, rsem.at[sem],
                                         device_id=(tx, ty), device_id_type=MESH).start()

        def wait_recv(e):
            pltpu.make_async_copy(rbuf.at[e], rbuf.at[e], rsem.at[e]).wait()

        def step(s, _):
            u, n = s // NT, s % NT
            m, odd, kb, jb = coords(u)
            slot = u % NSLOT
            lhs = kb + 2 * odd
            dst = jb + 2 - 2 * odd

            r = s + LAG
            pl.when(r < NREG)(lambda: issue(r))
            pl.when(jnp.logical_and(r >= NREG, r < NREG + TLAG))(lambda: issue_tail(r - NREG))

            @pl.when(n == 0)
            def _():
                @pl.when(jnp.logical_and(jb == 0, m > 0))
                def _():
                    e = (m - 1) // 2 * 6 + 4 - 4 * odd + kb
                    wait_recv(e)
                    lo = jnp.where(odd == 1, 0.0, -jnp.inf)
                    for t in range(NT):
                        v = acc[lhs, t] + rbuf[e, t].astype(jnp.float32)
                        act[lhs, :, t * LANES:(t + 1) * LANES] = jnp.maximum(v, lo).astype(act.dtype)
                pltpu.make_async_copy(wbuf.at[slot], wbuf.at[slot], wsem.at[slot]).wait()

            if compute:
                p = mm(lhs, slot, n)
            else:
                p = jnp.zeros((B, LANES), jnp.float32)

            @pl.when(kb == 0)
            def _():
                acc[dst, n] = p

            @pl.when(kb > 0)
            def _():
                v = acc[dst, n] + p
                acc[dst, n] = v

                @pl.when(kb == 1 + 2 * odd)
                def _():
                    e = m // 2 * 6 + 4 * odd + jb
                    sbuf[e, n] = v.astype(jnp.bfloat16)
                    send(e, n, e, odd)

        lax.fori_loop(0, NREG, step, None)

        wait_recv(16)
        for t in range(NT):
            obuf[:, t * LANES:(t + 1) * LANES] = acc[0, t] + rbuf[16, t].astype(jnp.float32)

        def tail(q, _):
            n, hh = q // 2, q % 2
            slot = (NUNIT - 2 + hh) % NSLOT
            pl.when(q + TLAG < 2 * NT)(lambda: issue_tail(q + TLAG))
            strip = wbuf.at[slot, :, pl.ds(pl.multiple_of(n * LANES, LANES), LANES)]
            pltpu.make_async_copy(strip, strip, tsem.at[q]).wait()
            v = acc[1, n] + mm(4 + hh, slot, n)
            acc[1, n] = v

            @pl.when(hh == 1)
            def _():
                sbuf[17, n] = v.astype(jnp.bfloat16)
                send(17, n, 17 + n, 1)

        lax.fori_loop(0, 2 * NT, tail, None)

        for n in range(NT):
            pltpu.make_async_copy(rbuf.at[17, n], rbuf.at[17, n], rsem.at[17 + n]).wait()
            obuf[:, U + n * LANES:U + (n + 1) * LANES] = acc[1, n] + rbuf[17, n].astype(jnp.float32)
        pltpu.make_async_copy(sbuf, sbuf, ssem).wait()

    def fn(x, Win0, Wout0, Win1, Wout1, Win2, Wout2):
        hbm = pl.BlockSpec(memory_space=pltpu.HBM)
        return pl.pallas_call(
            body,
            out_shape=jax.ShapeDtypeStruct(x.shape, jnp.float32),
            in_specs=[hbm] * 7,
            out_specs=pl.BlockSpec(memory_space=pltpu.VMEM),
            scratch_shapes=[
                pltpu.VMEM((NSLOT, U, U), jnp.float32),
                pltpu.VMEM((6, B, U), jnp.float32 if f32mm else jnp.bfloat16),
                pltpu.VMEM((6, NT, B, LANES), jnp.float32),
                pltpu.VMEM((18, NT, B, LANES), jnp.bfloat16),
                pltpu.VMEM((18, NT, B, LANES), jnp.bfloat16),
                pltpu.VMEM((B, 2 * U), jnp.float32),
                pltpu.SemaphoreType.DMA((NSLOT,)),
                pltpu.SemaphoreType.DMA((2 * NT,)),
                pltpu.SemaphoreType.DMA,
                pltpu.SemaphoreType.DMA,
                pltpu.SemaphoreType.DMA((17 + NT,)),
            ],
            compiler_params=pltpu.CompilerParams(
                vmem_limit_bytes=64 * 2**20, collective_id=0,
                disable_bounds_checks=not checks),
        )(x, Win0, Wout0, Win1, Wout1, Win2, Wout2)
    return fn


def pallas_dist_mlpseq_tp2d_cs_cs_b64_d2048_h4096_kernel(x, Win0, Wout0, Win1, Wout1, Win2, Wout2):
    return make()(x, Win0, Wout0, Win1, Wout1, Win2, Wout2)
```

```python
import jax
import jax.numpy as jnp
from jax import lax
from jax.experimental import pallas as pl
from jax.experimental.pallas import tpu as pltpu

MESH = pl.DeviceIdType.MESH
B = 64
LANES = 128
SUB = 8
NT = 8
KR = 128
WT = 8192
O = 7


def tiles(w):
    r, c = w.shape
    return w.reshape(r // SUB, SUB, c // LANES, LANES).transpose(0, 2, 1, 3)


def span(basis):
    out = [0]
    for v in basis:
        out = out + [z ^ v for z in out]
    return out


def make(checks=False, semcheck=False, kbasis=(16, 1, 32, 64), jbasis=(128, 2, 4, 8), sorder=None,
         tailcomm=True, shift=4, ahead=1, ksplit=0, xpieces=4, worder=None):
    sorder = sorder or [4 * s + t for t in range(4) for s in range(4)]
    worder = worder or list(range(16))
    KV = span(kbasis)

    def body(x_hbm, w0, w1, w2, w3, w4, w5, w5s, obuf,
             wbuf, tbuf, act, acc, sbuf, rbuf, xf,
             wsem, tsem, xsem, ssem, rsem):
        ws = (w0, w1, w2, w3, w4, w5)

        def load(m, f, n, sem, prio):
            pltpu.make_async_copy(ws[m].at[pl.ds(f, n)], wbuf.at[m % 2, pl.ds(f, n)], wsem.at[sem]).start(priority=prio)

        def issue_pairs(m, j):
            base = (j >> 4) * 256
            for i, v in enumerate(jbasis):
                base = base + ((j >> i) & 1) * v
            f0 = base * NT + O
            sem = (j >> 4) if m % 2 else (j >> 5)
            sem = sem + 4 * (m % 2)
            for k, v in enumerate(KV):
                f = f0 + v * NT
                if m < 5 and v == max(KV):
                    pl.when(j < 63)(lambda: load(m, f, NT, sem, k % 2))

                    @pl.when(j == 63)
                    def _():
                        load(m, WT - NT + O, NT - O, sem, k % 2)
                        load(m + 1, 0, O, sem, k % 2)
                else:
                    load(m, f, NT, sem, k % 2)

        def issue_wrap(j):
            kb, i = j >> 3, j & 7
            f0 = (kb * KR + i) * 16 + O + NT
            for k, s in enumerate(worder):
                f = f0 + s * 8 * 16
                if s == 15:
                    pl.when(j < 31)(lambda: load(5, f, NT, 4 + kb, k % 2))
                    pl.when(j == 31)(lambda: load(5, WT - NT + O, NT - O, 4 + kb, k % 2))
                else:
                    load(5, f, NT, 4 + kb, k % 2)

        def mid_item(d, prio):
            if d < 128:
                load(5, (2 * KR + d // 16 + worder[d % 16] * 8) * 16 + O, NT, 0, prio)
            else:
                q, k = (d - 128) // 16, d % 16
                s, sem = sorder[k], q
                if ksplit and q == 7:
                    s = k
                    sem = 8 if k >= 16 - ksplit else 7
                pltpu.make_async_copy(w5s.at[pl.ds(3 * KR + s * 8, 8), O + q], tbuf.at[q, pl.ds(s * 8, 8)],
                                      tsem.at[sem]).start(priority=prio)

        def issue_mid(j):
            sh = 8 * shift
            for i in range(8 * j, 8 * j + 8):
                mid_item(i if i < sh else 2 * i - sh + (1 if sh else 0), 0)
                mid_item(sh + 2 * i + (0 if sh else 1) if i < 128 - sh else 128 + i, 1)

        issue_pairs(0, jnp.int32(0))
        load(0, 0, O, 4, 0)

        mx = lax.axis_index("x")
        my = lax.axis_index("y")
        bsem = pltpu.get_barrier_semaphore()
        pl.semaphore_signal(bsem, 1, device_id=(1 - mx, my), device_id_type=MESH)
        pl.semaphore_signal(bsem, 1, device_id=(mx, 1 - my), device_id_type=MESH)
        x_copy = pltpu.make_async_copy(x_hbm, xf, xsem)
        pl.when(mx == 0)(x_copy.start)

        def mm(a, w):
            w = w.reshape(w.shape[0] * SUB, LANES).astype(jnp.bfloat16)
            return jnp.dot(a, w, preferred_element_type=jnp.float32)

        def send(t, sem, odd):
            tx = jnp.where(odd == 1, 1 - mx, mx)
            ty = jnp.where(odd == 1, my, 1 - my)
            pltpu.make_async_remote_copy(sbuf.at[t], rbuf.at[t], ssem, rsem.at[sem],
                                         device_id=(tx, ty), device_id_type=MESH).start()

        def wait_recv(t0, n, sem):
            r = rbuf.at[pl.ds(t0, n)]
            pltpu.make_async_copy(r, r, rsem.at[sem]).wait()

        def wait_w(n, sem):
            r = wbuf.at[0, pl.ds(0, n)]
            pltpu.make_async_copy(r, r, wsem.at[sem]).wait()

        def step(s, _):
            m, t = s >> 6, s & 63
            odd = m & 1
            wrap = s >= 352
            kb = jnp.where(wrap, (s - 336) >> 3, t >> (5 - odd))
            n = jnp.where(wrap, s & 7, t & (31 >> odd))
            c = jnp.where(wrap, (n + O + NT) & 15, n)
            lhs = kb + 2 * odd
            dst = c + (16 - 16 * odd)

            @pl.when(n == 0)
            def _():
                @pl.when(m > 0)
                def _():
                    e = ((m - 1) >> 1) * 6 + 4 - 4 * odd + kb
                    wait_recv(e * NT, NT, e)
                    lo = jnp.where(odd == 1, 0.0, -jnp.inf)
                    for i in range(NT):
                        v = acc[lhs * NT + i] + rbuf[e * NT + i].astype(jnp.float32)
                        act[lhs, :, i * LANES:(i + 1) * LANES] = jnp.maximum(v, lo).astype(act.dtype)

                sem = kb + 4 * odd
                pl.when(odd == 0)(lambda: wait_w(4096, sem))
                pl.when((odd == 1) & (s < 352))(lambda: wait_w(2048, sem))
                pl.when(s == 352)(lambda: wait_w(1024, sem))
                pl.when(s == 360)(lambda: wait_w(1024 - O, sem))

            @pl.when(kb == 0)
            def _():
                acc[dst] = jnp.zeros((B, LANES), jnp.float32)

            def go(p, w):
                acc[dst] = acc[dst] + mm(act[lhs], wbuf[p, pl.ds(kb * KR * w + c, KR, stride=w)])
            pl.when(odd == 0)(lambda: go(0, 32))
            pl.when(odd == 1)(lambda: go(1, 16))

            @pl.when(kb == 1 + 2 * odd)
            def _():
                e = (m >> 1) * 48 + 32 * odd + c
                sbuf[e] = acc[dst].astype(jnp.bfloat16)
                if tailcomm:
                    send(e, e >> 3, odd)
                else:
                    pl.when(m < 5)(lambda: send(e, e >> 3, odd))

        def steps_before(r):
            def seg(lo, hi):
                return jnp.clip(r - lo, 0, hi - lo)
            return seg(38, 378) + seg(326, 342) + seg(358, 366) + seg(374, 378)

        XP = 2 * xpieces
        XR = B // xpieces

        def share_x(i):
            r = act.at[i // xpieces, pl.ds(pl.multiple_of(i % xpieces * XR, XR), XR)]
            return pltpu.make_async_remote_copy(r, r, xsem, rsem.at[26], device_id=(1 - mx, my), device_id_type=MESH)

        def tick(r, _):
            m, j = r >> 6, r & 63
            for k in range(5):
                pl.when(m == k)(lambda k=k: issue_pairs(k, j))
            pl.when((m == 5) & (j < 32))(lambda: issue_pairs(5, j))
            pl.when((m == 5) & (j >= 32))(lambda: issue_wrap(j - 16))

            @pl.when(r < 38)
            def _():
                @pl.when(r == 12)
                def _():
                    wait_w(O, 4)
                    pl.semaphore_wait(bsem, 2)

                    @pl.when(mx == 0)
                    def _():
                        x_copy.wait()
                        for b in range(2):
                            act[b] = xf[:, b * 1024:(b + 1) * 1024].astype(act.dtype)

                pl.when((mx == 0) & (r >= 12) & (r < 12 + XP))(lambda: share_x(r - 12).start())

                @pl.when(r == 37)
                def _():
                    both = act.at[pl.ds(0, 2)]
                    pl.when(mx == 0)(pltpu.make_async_copy(both, both, xsem).wait)
                    pl.when(mx == 1)(pltpu.make_async_copy(both, both, rsem.at[26]).wait)

            lax.fori_loop(steps_before(r), steps_before(r + 1), step, None)

        lax.fori_loop(1, 368, tick, None)

        def tick2(r, _):
            for j in range(10):
                pl.when(r == 368 + j)(lambda j=j: issue_mid(j))
            lax.fori_loop(steps_before(r), steps_before(r + 1), step, None)

        lax.fori_loop(368, 378, tick2, None)
        first = 8 + max(shift, 0) // 2 if shift else 12
        for j in range(10, first + ahead):
            issue_mid(j)
        wait_w(1024, 0)

        def tail(q, _):
            for j in range(first + ahead, 16):
                pl.when(q == j - first - ahead)(lambda j=j: issue_mid(j))
            c = O + q
            v = acc[c] + mm(act[4], wbuf[1, pl.ds(2 * KR * 16 + c, KR, stride=16)])
            pltpu.make_async_copy(tbuf.at[q], tbuf.at[q], tsem.at[q]).wait()
            v = v + mm(act[5], tbuf[q])
            acc[c] = v
            sbuf[128 + c] = v.astype(jnp.bfloat16)
            if tailcomm:
                send(128 + c, 18 + q, 1)

        if ksplit:
            lax.fori_loop(0, 7, tail, None)
            c, h = O + 7, KR - 8 * ksplit
            v = acc[c] + mm(act[4], wbuf[1, pl.ds(2 * KR * 16 + c, KR, stride=16)])
            pltpu.make_async_copy(tbuf.at[7, :h], tbuf.at[7, :h], tsem.at[7]).wait()
            v = v + mm(act[5, :, :h * SUB], tbuf[7, :h])
            pltpu.make_async_copy(tbuf.at[7, h:], tbuf.at[7, h:], tsem.at[8]).wait()
            v = v + mm(act[5, :, h * SUB:], tbuf[7, h:])
            sbuf[128 + c] = v.astype(jnp.bfloat16)
            if tailcomm:
                send(128 + c, 18 + 7, 1)
            acc[c] = v
        else:
            lax.fori_loop(0, 8, tail, None)

        def finish(c):
            obuf[:, c * LANES:(c + 1) * LANES] = acc[c] + rbuf[128 + c].astype(jnp.float32)

        if tailcomm:
            wait_recv(128, O, 16)
            wait_recv(128 + O + NT, NT - O, 17)
        for c in list(range(O)) + list(range(O + NT, 16)):
            finish(c)
        for q in range(8):
            if tailcomm:
                if q == 7:
                    pltpu.make_async_copy(sbuf, sbuf, ssem).wait()
                wait_recv(128 + O + q, 1, 18 + q)
            finish(O + q)
        if not tailcomm:
            pltpu.make_async_copy(sbuf.at[:128], sbuf.at[:128], ssem).wait()

    def fn(x, *ws):
        hbm = pl.BlockSpec(memory_space=pltpu.HBM)
        flat = [tiles(w).reshape(WT, SUB, LANES) for w in ws]
        return pl.pallas_call(
            body,
            out_shape=jax.ShapeDtypeStruct(x.shape, jnp.float32),
            in_specs=[hbm] * 8,
            out_specs=pl.BlockSpec(memory_space=pltpu.VMEM),
            scratch_shapes=[
                pltpu.VMEM((2, WT, SUB, LANES), jnp.float32),
                pltpu.VMEM((8, KR, SUB, LANES), jnp.float32),
                pltpu.VMEM((6, B, 1024), jnp.bfloat16),
                pltpu.VMEM((6 * NT, B, LANES), jnp.float32),
                pltpu.VMEM((18 * NT, B, LANES), jnp.bfloat16),
                pltpu.VMEM((18 * NT, B, LANES), jnp.bfloat16),
                pltpu.VMEM((B, 2048), jnp.float32),
                pltpu.SemaphoreType.DMA((8,)),
                pltpu.SemaphoreType.DMA((9,)),
                pltpu.SemaphoreType.DMA,
                pltpu.SemaphoreType.DMA,
                pltpu.SemaphoreType.DMA((27,)),
            ],
            compiler_params=pltpu.CompilerParams(
                vmem_limit_bytes=96 * 2**20, collective_id=0,
                disable_bounds_checks=not checks, disable_semaphore_checks=not semcheck),
        )(x, *flat, tiles(ws[5]))
    return fn


def pallas_dist_mlpseq_tp2d_cs_cs_b64_d2048_h4096_kernel(x, Win0, Wout0, Win1, Wout1, Win2, Wout2):
    return make(ksplit=4)(x, Win0, Wout0, Win1, Wout1, Win2, Wout2)
```

```python
import functools

import jax
import jax.numpy as jnp
from jax import lax
from jax.experimental import pallas as pl
from jax.experimental.pallas import tpu as pltpu

BATCH = 64
SUB, LANES = 8, 128
TILES = 8192
WIDTH = (32, 16)
KROWS = 128
KBLK = KROWS * SUB
BLK = 8
PHASE = 7
LAST_BLOCK = TILES // BLK - 1


def _span(basis):
    out = [0]
    for v in basis:
        out = out + [z ^ v for z in out]
    return out


ROUND_BLOCKS = _span((16, 1, 32, 64))
ROUND_STRIDES = (128, 2, 4, 8, 256, 512)
COLUMN_ROWS = _span((42, 17, 32, 64))
STRIP_PIECES = _span((8, 1, 2, 4))
STRIP_STAGES = ((0, 2), (1, 3), (4, 6), (5,))
LAST_STRIP = 7
LAST_EARLY = 80
QUEUE = 32
AHEAD, DRIP = 6, 3

WARM_UP = 38
HALF_ROUND = 352
END_ROUND = 368
LOOP_ROUNDS = 378
HALF_STEP = 352


def _steps_before(r):
    def rounds(lo, hi):
        return jnp.clip(r - lo, 0, hi - lo)
    return rounds(WARM_UP, LOOP_ROUNDS) + rounds(326, 342) + rounds(358, 366) + rounds(374, 378)


def _as_tiles(w):
    rows, cols = w.shape
    return w.reshape(rows // SUB, SUB, cols // LANES, LANES).transpose(0, 2, 1, 3)


def _body(x_hbm, w0, w1, w2, w3, w4, w5, w5_rows, w5_comb, out_ref,
          win_buf, wout_buf, strip_buf, last_buf, x_buf, act, acc, send_buf, recv_buf,
          head_sem, group_sem, strip_sem, x_sem, share_sem, send_sem, recv_sem):
    weights = (w0, w1, w2, w3, w4, w5)
    bufs = (win_buf, wout_buf)

    def wait_for(ref, sem):
        pltpu.make_async_copy(ref, ref, sem).wait()

    def head(odd):
        return bufs[odd].at[0, pl.ds(WIDTH[odd] - PHASE, PHASE)]

    def load_head(m):
        pltpu.make_async_copy(weights[m].at[pl.ds(0, PHASE)], head(m % 2), head_sem.at[m % 2]).start()

    def load_block(m, p, sem, thread, n=BLK):
        per_row = WIDTH[m % 2] // BLK
        row = 1 + (p >> (per_row.bit_length() - 1))
        col = (p & (per_row - 1)) * BLK
        pltpu.make_async_copy(weights[m].at[pl.ds(PHASE + BLK * p, n)],
                              bufs[m % 2].at[row, pl.ds(col, n)], sem).start(priority=thread)

    def load_maybe_last_block(m, p, sem, thread):
        pl.when(p < LAST_BLOCK)(lambda: load_block(m, p, sem, thread))

        @pl.when(p == LAST_BLOCK)
        def _():
            load_block(m, LAST_BLOCK, sem, thread, BLK - PHASE)
            width = WIDTH[m % 2]
            rest = bufs[m % 2].at[TILES // width, pl.ds(width - PHASE, PHASE)]
            pltpu.make_async_copy(head(m % 2), rest, sem).start()

    def load_round(m, j):
        base = sum(((j >> i) & 1) * v for i, v in enumerate(ROUND_STRIDES))
        sem = group_sem.at[4 + (j >> 4) if m % 2 else j >> 5]
        for k, v in enumerate(ROUND_BLOCKS):
            load = load_maybe_last_block if v == max(ROUND_BLOCKS) else load_block
            load(m, base + v, sem, k % 2)

    def load_odd_blocks(j):
        kb, i = j >> 3, j & 7
        for k, v in enumerate(COLUMN_ROWS):
            load = load_maybe_last_block if v >= KROWS - 8 else load_block
            load(5, 2 * (kb * KROWS + (v ^ i)) + 1, group_sem.at[4 + kb], k % 2)

    def load_strip(q, s, thread):
        pltpu.make_async_copy(w5_comb.at[pl.ds(3 * KROWS // 16, 8), s, PHASE + q],
                              strip_buf.at[q, :, s], strip_sem.at[q]).start(priority=thread)

    def load_last_strip(r, thread):
        sem = strip_sem.at[LAST_STRIP if r < LAST_EARLY else BLK]
        pltpu.make_async_copy(w5_rows.at[pl.ds(3 * KROWS + r, 8), PHASE + LAST_STRIP],
                              last_buf.at[pl.ds(r, 8)], sem).start(priority=thread)

    ending = [functools.partial(load_block, 5, 2 * (2 * KROWS + (v ^ i)), group_sem.at[0])
              for i in range(8) for v in COLUMN_ROWS]
    stage_ends = [len(ending)]
    for stage in STRIP_STAGES:
        ending += [functools.partial(load_strip, q, s) for s in STRIP_PIECES for q in stage]
        stage_ends.append(len(ending))
    ending += [functools.partial(load_last_strip, r) for r in range(0, KROWS, 8)]
    pairs = len(ending) // 2

    def load_ending(lo, hi):
        for i in range(lo, min(hi, pairs)):
            ending[i if i < QUEUE else 2 * i - QUEUE + 1](0)
            ending[QUEUE + 2 * i if i < pairs - QUEUE else pairs + i](1)

    for base in (0, ROUND_STRIDES[0]):
        for v in ROUND_BLOCKS:
            load_block(0, base + v, group_sem.at[0], 1)
    load_head(0)

    mx, my = lax.axis_index("x"), lax.axis_index("y")

    def remote_copy(src, dst, sent, received, along_x):
        return pltpu.make_async_remote_copy(
            src, dst, sent, received, device_id=(mx ^ along_x, my ^ (1 - along_x)),
            device_id_type=pl.DeviceIdType.MESH)

    barrier = pltpu.get_barrier_semaphore()
    for partner in ((1 - mx, my), (mx, 1 - my)):
        pl.semaphore_signal(barrier, 1, device_id=partner, device_id_type=pl.DeviceIdType.MESH)

    pl.when(mx == 0)(lambda: pltpu.make_async_copy(x_hbm, x_buf, x_sem).start())

    def share_x(ref):
        return remote_copy(ref, ref, share_sem.at[0], share_sem.at[1], 1)

    def start_up(r):
        @pl.when(r == 12)
        def _():
            pl.semaphore_wait(barrier, 2)

            @pl.when(mx == 0)
            def _():
                pltpu.make_async_copy(x_hbm, x_buf, x_sem).wait()
                for b in range(2):
                    act[b] = x_buf[:, b * KBLK:(b + 1) * KBLK].astype(act.dtype)

        @pl.when((mx == 0) & (r >= 12) & (r < 20))
        def _():
            i = r - 12
            share_x(act.at[i >> 2, pl.ds(pl.multiple_of((i & 3) * 16, 16), 16)]).start()

        @pl.when(r == WARM_UP - 1)
        def _():
            x_bf16 = act.at[pl.ds(0, 2)]
            pl.when(mx == 0)(lambda: share_x(x_bf16).wait_send())
            pl.when(mx == 1)(lambda: share_x(x_bf16).wait_recv())

    def matmul(a, w_tiles):
        w = w_tiles.reshape(a.shape[1], LANES).astype(jnp.bfloat16)
        return jnp.dot(a, w, preferred_element_type=jnp.float32)

    def send(slot, partial, sem, along_x):
        send_buf[slot] = partial.astype(send_buf.dtype)
        remote_copy(send_buf.at[slot], recv_buf.at[slot], send_sem, recv_sem.at[sem], along_x).start()

    def step(s, _):
        m, t = s >> 6, s & 63
        odd = m & 1
        half = s >= HALF_STEP
        kb = jnp.where(half, 2 + ((s - HALF_STEP) >> 3), t >> (5 - odd))
        n = jnp.where(half, s & 7, t & (31 >> odd))
        c = jnp.where(half, (PHASE + BLK + n) & 15, n)
        lhs = kb + 2 * odd
        dst = c + 16 * (1 - odd)

        @pl.when((n == 0) & (m > 0))
        def _():
            e = ((m - 1) >> 1) * 6 + 4 * (1 - odd) + kb
            wait_for(recv_buf.at[pl.ds(e * BLK, BLK)], recv_sem.at[e])

            def reduce(relu):
                for i in range(BLK):
                    v = acc[lhs * BLK + i] + recv_buf[e * BLK + i].astype(jnp.float32)
                    if relu:
                        v = jnp.maximum(v, 0.0)
                    act[lhs, :, i * LANES:(i + 1) * LANES] = v.astype(act.dtype)

            pl.when(odd == 1)(lambda: reduce(True))
            pl.when(odd == 0)(lambda: reduce(False))

        @pl.when(n == 0)
        def _():
            rows = pl.ds(1 + kb * KROWS, KROWS)
            sem = group_sem.at[kb + 4 * odd]
            for p in range(2):
                pl.when((odd == p) & (kb == 0))(lambda: wait_for(head(p), head_sem.at[p]))
                pl.when((odd == p) & (s < HALF_STEP))(lambda: wait_for(bufs[p].at[rows], sem))
            pl.when(half)(lambda: wait_for(wout_buf.at[rows, pl.ds(BLK, BLK)], sem))

        @pl.when(kb == 0)
        def _():
            acc[dst] = jnp.zeros((BATCH, LANES), jnp.float32)

        for p in range(2):
            @pl.when(odd == p)
            def _():
                row = kb * KROWS + jnp.where(c >= PHASE, 1, 0)
                col = (c + WIDTH[p] - PHASE) & (WIDTH[p] - 1)
                acc[dst] = acc[dst] + matmul(act[lhs], bufs[p][pl.ds(row, KROWS), col])

        @pl.when(kb == 1 + 2 * odd)
        def _():
            slot = (m >> 1) * 48 + 32 * odd + c
            send(slot, acc[dst], slot >> 3, odd)

    def run_round(r, _):
        m, j = r >> 6, r & 63
        for k in range(5):
            @pl.when(m == k)
            def _():
                load_round(k, j)
                pl.when(j == 63)(lambda: load_head(k + 1))

        pl.when((m == 5) & (r < HALF_ROUND))(lambda: load_round(5, j))
        pl.when((r >= HALF_ROUND) & (r < END_ROUND))(lambda: load_odd_blocks(r - HALF_ROUND + 16))

        @pl.when(r >= END_ROUND)
        def _():
            for i in range(LOOP_ROUNDS - END_ROUND):
                pl.when(r == END_ROUND + i)(lambda: load_ending(8 * i, 8 * i + 8))

        pl.when(r < WARM_UP)(lambda: start_up(r))
        lax.fori_loop(_steps_before(r), _steps_before(r + 1), step, None)

    lax.fori_loop(2, LOOP_ROUNDS, run_round, None)

    out_slots = 16 * BLK
    started = 8 * (LOOP_ROUNDS - END_ROUND)

    def load_until(pair):
        nonlocal started
        load_ending(started, pair)
        started = max(started, pair)

    def third_group(q):
        return matmul(act[4], wout_buf[pl.ds(1 + 2 * KROWS, KROWS), q])

    def send_out(q, partial):
        send(out_slots + PHASE + q, partial, 18 + q, 1)
        acc[PHASE + q] = partial

    load_until((stage_ends[0] + QUEUE) // 2 + AHEAD)
    wait_for(wout_buf.at[pl.ds(1 + 2 * KROWS, KROWS), pl.ds(0, BLK)], group_sem.at[0])
    for stage, end in zip(STRIP_STAGES, stage_ends[1:]):
        load_until((end + QUEUE) // 2 + AHEAD)
        for q in stage:
            acc[PHASE + q] = acc[PHASE + q] + third_group(q)
        for q in stage:
            wait_for(strip_buf.at[q], strip_sem.at[q])
            send_out(q, acc[PHASE + q] + matmul(act[5], strip_buf[q]))
            load_until(started + DRIP)
    load_until(pairs)

    early = LAST_EARLY
    partial = acc[PHASE + LAST_STRIP] + third_group(LAST_STRIP)
    wait_for(last_buf.at[:early], strip_sem.at[LAST_STRIP])
    partial = partial + matmul(act[5, :, :early * SUB], last_buf[:early])
    wait_for(last_buf.at[early:], strip_sem.at[BLK])
    send_out(LAST_STRIP, partial + matmul(act[5, :, early * SUB:], last_buf[early:]))

    def finish(c):
        total = acc[c] + recv_buf[out_slots + c].astype(jnp.float32)
        out_ref[:, c * LANES:(c + 1) * LANES] = total

    def finish_strip(q):
        wait_for(recv_buf.at[out_slots + PHASE + q], recv_sem.at[18 + q])
        finish(PHASE + q)

    wait_for(recv_buf.at[out_slots:out_slots + PHASE], recv_sem.at[16])
    wait_for(recv_buf.at[out_slots + PHASE + BLK:], recv_sem.at[17])
    for c in (*range(PHASE), *range(PHASE + BLK, WIDTH[1])):
        finish(c)
    for stage in STRIP_STAGES:
        for q in stage:
            finish_strip(q)
    remote_copy(send_buf, recv_buf, send_sem, recv_sem.at[0], 1).wait_send()
    finish_strip(LAST_STRIP)


def pallas_dist_mlpseq_tp2d_cs_cs_b64_d2048_h4096_kernel(
    x: jax.Array,
    Win0: jax.Array,
    Wout0: jax.Array,
    Win1: jax.Array,
    Wout1: jax.Array,
    Win2: jax.Array,
    Wout2: jax.Array,
):
    tiled = [_as_tiles(w) for w in (Win0, Wout0, Win1, Wout1, Win2, Wout2)]
    dma_sems = pltpu.SemaphoreType.DMA
    return pl.pallas_call(
        _body,
        out_shape=jax.ShapeDtypeStruct(x.shape, jnp.float32),
        in_specs=[pl.BlockSpec(memory_space=pltpu.HBM)] * 9,
        out_specs=pl.BlockSpec(memory_space=pltpu.VMEM),
        scratch_shapes=[
            pltpu.VMEM((TILES // WIDTH[0] + 1, WIDTH[0], SUB, LANES), jnp.float32),
            pltpu.VMEM((TILES // WIDTH[1] + 1, WIDTH[1], SUB, LANES), jnp.float32),
            pltpu.VMEM((BLK - 1, 8, 16, SUB, LANES), jnp.float32),
            pltpu.VMEM((KROWS, SUB, LANES), jnp.float32),
            pltpu.VMEM(x.shape, jnp.float32),
            pltpu.VMEM((6, BATCH, KBLK), jnp.bfloat16),
            pltpu.VMEM((48, BATCH, LANES), jnp.float32),
            pltpu.VMEM((3 * 48, BATCH, LANES), jnp.bfloat16),
            pltpu.VMEM((3 * 48, BATCH, LANES), jnp.bfloat16),
            dma_sems((2,)),
            dma_sems((8,)),
            dma_sems((BLK + 1,)),
            dma_sems,
            dma_sems((2,)),
            dma_sems,
            dma_sems((18 + BLK,)),
        ],
        compiler_params=pltpu.CompilerParams(
            collective_id=0,
            vmem_limit_bytes=96 * 2**20,
            disable_bounds_checks=True,
            disable_semaphore_checks=True,
        ),
    )(
        x,
        *[t.reshape(TILES, SUB, LANES) for t in tiled],
        tiled[5],
        tiled[5].reshape(32, 16, WIDTH[1], SUB, LANES),
    )
```

```python
import functools

import jax
import jax.numpy as jnp
from jax import lax
from jax.experimental import pallas as pl
from jax.experimental.pallas import tpu as pltpu

BATCH = 64
SUB, LANES = 8, 128
TILES = 8192
WIDTH = (32, 16)
KROWS = 128
KBLK = KROWS * SUB
BLK = 8
PHASE = 7
LAST_BLOCK = TILES // BLK - 1


def _span(basis):
    out = [0]
    for v in basis:
        out = out + [z ^ v for z in out]
    return out


ROUND_BLOCKS = _span((16, 1, 32, 64))
ROUND_STRIDES = (128, 2, 4, 8, 256, 512)
COLUMN_ROWS = _span((42, 17, 32, 64))
STRIP_PIECES = _span((8, 1, 2, 4))
STRIP_STAGES = ((0, 2), (1, 3), (4, 6), (5,))
LAST_STRIP = 7
LAST_EARLY = 64
QUEUE = 30
AHEAD, DRIP = 6, 3

WARM_UP = 38
HALF_ROUND = 352
END_ROUND = 368
LOOP_ROUNDS = 378
HALF_STEP = 352


def _steps_before(r):
    def rounds(lo, hi):
        return jnp.clip(r - lo, 0, hi - lo)
    return rounds(WARM_UP, LOOP_ROUNDS) + (rounds(326, 374) >> 1) + rounds(374, LOOP_ROUNDS)


def _as_tiles(w):
    rows, cols = w.shape
    return w.reshape(rows // SUB, SUB, cols // LANES, LANES).transpose(0, 2, 1, 3)


def _body(x_hbm, w0, w1, w2, w3, w4, w5, w5_rows, w5_comb, out_ref,
          win_buf, wout_buf, strip_buf, last_buf, x_buf, act, acc, send_buf, recv_buf,
          head_sem, group_sem, strip_sem, x_sem, share_sem, send_sem, recv_sem):
    weights = (w0, w1, w2, w3, w4, w5)
    bufs = (win_buf, wout_buf)

    def wait_for(ref, sem):
        pltpu.make_async_copy(ref, ref, sem).wait()

    def head(odd):
        return bufs[odd].at[0, pl.ds(WIDTH[odd] - PHASE, PHASE)]

    def load_head(m):
        pltpu.make_async_copy(weights[m].at[pl.ds(0, PHASE)], head(m % 2), head_sem.at[m % 2]).start()

    def load_block(m, p, sem, thread, n=BLK):
        per_row = WIDTH[m % 2] // BLK
        row = 1 + (p >> (per_row.bit_length() - 1))
        col = (p & (per_row - 1)) * BLK
        pltpu.make_async_copy(weights[m].at[pl.ds(PHASE + BLK * p, n)],
                              bufs[m % 2].at[row, pl.ds(col, n)], sem).start(priority=thread)

    def load_maybe_last_block(m, p, sem, thread):
        pl.when(p < LAST_BLOCK)(lambda: load_block(m, p, sem, thread))

        @pl.when(p == LAST_BLOCK)
        def _():
            load_block(m, LAST_BLOCK, sem, thread, BLK - PHASE)
            width = WIDTH[m % 2]
            rest = bufs[m % 2].at[TILES // width, pl.ds(width - PHASE, PHASE)]
            pltpu.make_async_copy(head(m % 2), rest, sem).start()

    def load_round(m, j):
        base = sum(((j >> i) & 1) * v for i, v in enumerate(ROUND_STRIDES))
        sem = group_sem.at[4 + (j >> 4) if m % 2 else j >> 5]
        for k, v in enumerate(ROUND_BLOCKS):
            load = load_maybe_last_block if v == max(ROUND_BLOCKS) else load_block
            load(m, base + v, sem, k % 2)

    def load_odd_blocks(j):
        kb, i = j >> 3, j & 7
        for k, v in enumerate(COLUMN_ROWS):
            load = load_maybe_last_block if v >= KROWS - 8 else load_block
            load(5, 2 * (kb * KROWS + (v ^ i)) + 1, group_sem.at[4 + kb], k % 2)

    def load_strip(q, s, thread):
        pltpu.make_async_copy(w5_comb.at[pl.ds(3 * KROWS // 16, 8), s, PHASE + q],
                              strip_buf.at[q, :, s], strip_sem.at[q]).start(priority=thread)

    def load_last_strip(r, thread):
        sem = strip_sem.at[LAST_STRIP if r < LAST_EARLY else BLK]
        pltpu.make_async_copy(w5_rows.at[pl.ds(3 * KROWS + r, 8), PHASE + LAST_STRIP],
                              last_buf.at[pl.ds(r, 8)], sem).start(priority=thread)

    ending = [functools.partial(load_block, 5, 2 * (2 * KROWS + (v ^ i)), group_sem.at[0])
              for i in range(8) for v in COLUMN_ROWS]
    stage_ends = [len(ending)]
    for stage in STRIP_STAGES:
        ending += [functools.partial(load_strip, q, s) for s in STRIP_PIECES for q in stage]
        stage_ends.append(len(ending))
    ending += [functools.partial(load_last_strip, r) for r in range(0, KROWS, 8)]
    pairs = len(ending) // 2

    def load_ending(lo, hi):
        for i in range(lo, min(hi, pairs)):
            ending[i if i < QUEUE else 2 * i - QUEUE + 1](0)
            ending[QUEUE + 2 * i if i < pairs - QUEUE else pairs + i](1)

    for base in (0, ROUND_STRIDES[0]):
        for v in ROUND_BLOCKS:
            load_block(0, base + v, group_sem.at[0], 1)
    load_head(0)

    mx, my = lax.axis_index("x"), lax.axis_index("y")

    def remote_copy(src, dst, sent, received, along_x):
        return pltpu.make_async_remote_copy(
            src, dst, sent, received, device_id=(mx ^ along_x, my ^ (1 - along_x)),
            device_id_type=pl.DeviceIdType.MESH)

    barrier = pltpu.get_barrier_semaphore()
    for partner in ((1 - mx, my), (mx, 1 - my)):
        pl.semaphore_signal(barrier, 1, device_id=partner, device_id_type=pl.DeviceIdType.MESH)

    pl.when(mx == 0)(lambda: pltpu.make_async_copy(x_hbm, x_buf, x_sem).start())

    def share_x(ref):
        return remote_copy(ref, ref, share_sem.at[0], share_sem.at[1], 1)

    def start_up(r):
        @pl.when(r == 12)
        def _():
            pl.semaphore_wait(barrier, 2)

            @pl.when(mx == 0)
            def _():
                pltpu.make_async_copy(x_hbm, x_buf, x_sem).wait()
                for b in range(2):
                    act[b] = x_buf[:, b * KBLK:(b + 1) * KBLK].astype(act.dtype)

        @pl.when((mx == 0) & (r >= 12) & (r < 20))
        def _():
            i = r - 12
            share_x(act.at[i >> 2, pl.ds(pl.multiple_of((i & 3) * 16, 16), 16)]).start()

        @pl.when(r == WARM_UP - 1)
        def _():
            x_bf16 = act.at[pl.ds(0, 2)]
            pl.when(mx == 0)(lambda: share_x(x_bf16).wait_send())
            pl.when(mx == 1)(lambda: share_x(x_bf16).wait_recv())

    def matmul(a, w_tiles):
        w = w_tiles.reshape(a.shape[1], LANES).astype(jnp.bfloat16)
        return jnp.dot(a, w, preferred_element_type=jnp.float32)

    def send(slot, partial, sem, along_x, rows=BATCH):
        for lo in range(0, BATCH, rows):
            piece = pl.ds(lo, rows)
            send_buf[slot, piece] = partial[lo:lo + rows].astype(send_buf.dtype)
            remote_copy(send_buf.at[slot, piece], recv_buf.at[slot, piece],
                        send_sem, recv_sem.at[sem], along_x).start()

    def step(s, _):
        m, t = s >> 6, s & 63
        odd = m & 1
        half = s >= HALF_STEP
        kb = jnp.where(half, 2 + ((s - HALF_STEP) >> 3), t >> (5 - odd))
        n = jnp.where(half, s & 7, t & (31 >> odd))
        c = jnp.where(half, (PHASE + BLK + n) & 15, n)
        lhs = kb + 2 * odd
        dst = c + 16 * (1 - odd)

        @pl.when((n == 0) & (m > 0))
        def _():
            e = ((m - 1) >> 1) * 6 + 4 * (1 - odd) + kb
            wait_for(recv_buf.at[pl.ds(e * BLK, BLK)], recv_sem.at[e])

            def reduce(relu):
                for i in range(BLK):
                    v = acc[lhs * BLK + i] + recv_buf[e * BLK + i].astype(jnp.float32)
                    if relu:
                        v = jnp.maximum(v, 0.0)
                    act[lhs, :, i * LANES:(i + 1) * LANES] = v.astype(act.dtype)

            pl.when(odd == 1)(lambda: reduce(True))
            pl.when(odd == 0)(lambda: reduce(False))

        @pl.when(n == 0)
        def _():
            rows = pl.ds(1 + kb * KROWS, KROWS)
            sem = group_sem.at[kb + 4 * odd]
            for p in range(2):
                pl.when((odd == p) & (kb == 0))(lambda: wait_for(head(p), head_sem.at[p]))
                pl.when((odd == p) & (s < HALF_STEP))(lambda: wait_for(bufs[p].at[rows], sem))
            pl.when(half)(lambda: wait_for(wout_buf.at[rows, pl.ds(BLK, BLK)], sem))

        @pl.when(kb == 0)
        def _():
            acc[dst] = jnp.zeros((BATCH, LANES), jnp.float32)

        for p in range(2):
            @pl.when(odd == p)
            def _():
                row = kb * KROWS + jnp.where(c >= PHASE, 1, 0)
                col = (c + WIDTH[p] - PHASE) & (WIDTH[p] - 1)
                acc[dst] = acc[dst] + matmul(act[lhs], bufs[p][pl.ds(row, KROWS), col])

        @pl.when(kb == 1 + 2 * odd)
        def _():
            slot = (m >> 1) * 48 + 32 * odd + c
            send(slot, acc[dst], slot >> 3, odd)

    def run_round(r, _):
        m, j = r >> 6, r & 63
        for k in range(5):
            @pl.when(m == k)
            def _():
                load_round(k, j)
                pl.when(j == 63)(lambda: load_head(k + 1))

        pl.when((m == 5) & (r < HALF_ROUND))(lambda: load_round(5, j))
        pl.when((r >= HALF_ROUND) & (r < END_ROUND))(lambda: load_odd_blocks(r - HALF_ROUND + 16))

        @pl.when(r >= END_ROUND)
        def _():
            for lo in range(0, LOOP_ROUNDS - END_ROUND, 2):
                @pl.when((r - END_ROUND) >> 1 == lo >> 1)
                def _():
                    for i in (lo, lo + 1):
                        pl.when(r == END_ROUND + i)(lambda: load_ending(8 * i, 8 * i + 8))

        pl.when(r < WARM_UP)(lambda: start_up(r))
        lax.fori_loop(_steps_before(r), _steps_before(r + 1), step, None)

    lax.fori_loop(2, LOOP_ROUNDS, run_round, None)

    out_slots = 16 * BLK
    started = 8 * (LOOP_ROUNDS - END_ROUND)

    def load_until(pair):
        nonlocal started
        load_ending(started, pair)
        started = max(started, pair)

    def third_group(q):
        return matmul(act[4], wout_buf[pl.ds(1 + 2 * KROWS, KROWS), q])

    def send_out(q, partial, rows=BATCH):
        send(out_slots + PHASE + q, partial, 18 + q, 1, rows)
        acc[PHASE + q] = partial

    load_until((stage_ends[0] + QUEUE) // 2 + AHEAD)
    wait_for(wout_buf.at[pl.ds(1 + 2 * KROWS, KROWS), pl.ds(0, BLK)], group_sem.at[0])
    for stage, end in zip(STRIP_STAGES, stage_ends[1:]):
        load_until((end + QUEUE) // 2 + AHEAD)
        for q in stage:
            acc[PHASE + q] = acc[PHASE + q] + third_group(q)
        for q in stage:
            wait_for(strip_buf.at[q], strip_sem.at[q])
            send_out(q, acc[PHASE + q] + matmul(act[5], strip_buf[q]))
            load_until(started + DRIP)
    load_until(pairs)

    early = LAST_EARLY
    partial = acc[PHASE + LAST_STRIP] + third_group(LAST_STRIP)
    wait_for(last_buf.at[:early], strip_sem.at[LAST_STRIP])
    partial = partial + matmul(act[5, :, :early * SUB], last_buf[:early])
    wait_for(last_buf.at[early:], strip_sem.at[BLK])
    partial = partial + matmul(act[5, :, early * SUB:], last_buf[early:])
    send_out(LAST_STRIP, partial, rows=16)

    def finish(c):
        total = acc[c] + recv_buf[out_slots + c].astype(jnp.float32)
        out_ref[:, c * LANES:(c + 1) * LANES] = total

    def finish_strip(q):
        wait_for(recv_buf.at[out_slots + PHASE + q], recv_sem.at[18 + q])
        finish(PHASE + q)

    wait_for(recv_buf.at[out_slots:out_slots + PHASE], recv_sem.at[16])
    wait_for(recv_buf.at[out_slots + PHASE + BLK:], recv_sem.at[17])
    for c in (*range(PHASE), *range(PHASE + BLK, WIDTH[1])):
        finish(c)
    for stage in STRIP_STAGES:
        for q in stage:
            finish_strip(q)
    remote_copy(send_buf, send_buf, send_sem, recv_sem.at[0], 1).wait_send()
    finish_strip(LAST_STRIP)


def pallas_dist_mlpseq_tp2d_cs_cs_b64_d2048_h4096_kernel(
    x: jax.Array,
    Win0: jax.Array,
    Wout0: jax.Array,
    Win1: jax.Array,
    Wout1: jax.Array,
    Win2: jax.Array,
    Wout2: jax.Array,
):
    tiled = [_as_tiles(w) for w in (Win0, Wout0, Win1, Wout1, Win2, Wout2)]
    dma_sems = pltpu.SemaphoreType.DMA
    return pl.pallas_call(
        _body,
        out_shape=jax.ShapeDtypeStruct(x.shape, jnp.float32),
        in_specs=[pl.BlockSpec(memory_space=pltpu.HBM)] * 9,
        out_specs=pl.BlockSpec(memory_space=pltpu.VMEM),
        scratch_shapes=[
            pltpu.VMEM((TILES // WIDTH[0] + 1, WIDTH[0], SUB, LANES), jnp.float32),
            pltpu.VMEM((TILES // WIDTH[1] + 1, WIDTH[1], SUB, LANES), jnp.float32),
            pltpu.VMEM((BLK - 1, 8, 16, SUB, LANES), jnp.float32),
            pltpu.VMEM((KROWS, SUB, LANES), jnp.float32),
            pltpu.VMEM(x.shape, jnp.float32),
            pltpu.VMEM((6, BATCH, KBLK), jnp.bfloat16),
            pltpu.VMEM((48, BATCH, LANES), jnp.float32),
            pltpu.VMEM((3 * 48, BATCH, LANES), jnp.bfloat16),
            pltpu.VMEM((3 * 48, BATCH, LANES), jnp.bfloat16),
            dma_sems((2,)),
            dma_sems((8,)),
            dma_sems((BLK + 1,)),
            dma_sems,
            dma_sems((2,)),
            dma_sems,
            dma_sems((18 + BLK,)),
        ],
        compiler_params=pltpu.CompilerParams(
            collective_id=0,
            vmem_limit_bytes=96 * 2**20,
            disable_bounds_checks=True,
            disable_semaphore_checks=True,
        ),
    )(
        x,
        *[t.reshape(TILES, SUB, LANES) for t in tiled],
        tiled[5],
        tiled[5].reshape(32, 16, WIDTH[1], SUB, LANES),
    )
```
